```python
import numpy as np

kernel_name = "dist_mean_ax0_shard0_i_m2048_n1024"

def setup_inputs():
    return {"x": np.random.randn(8192, 1024).astype(np.float32)}

def reference(x: np.ndarray) -> np.ndarray:
    return np.mean(x, axis=0, keepdims=True)
```

```python
import jax
import jax.numpy as jnp
from jax import lax
from jax.experimental import pallas as pl
from jax.experimental.pallas import tpu as pltpu

N_DEV = 4
CHUNKS = (256, 256, 256, 256, 256, 256, 256, 128, 64, 64)


def pallas_dist_mean_ax0_shard0_i_m2048_n1024_kernel(
x: jax.Array,
):
    m_per, n = x.shape
    assert sum(CHUNKS) == m_per
    inv_total = 1.0 / float(m_per * N_DEV)

    def kernel_body(x_hbm, out_ref, xbuf, comm, copy_sems, send_sems, recv_sems):
        my = lax.axis_index("i")

        copies = []
        off = 0
        for c, rows in enumerate(CHUNKS):
            cp = pltpu.make_async_copy(
                x_hbm.at[pl.ds(off, rows)],
                xbuf.at[pl.ds(off, rows)],
                copy_sems.at[c],
            )
            cp.start()
            copies.append((cp, off, rows))
            off += rows

        barrier = pltpu.get_barrier_semaphore()
        for d in range(1, N_DEV):
            pl.semaphore_signal(
                barrier,
                inc=1,
                device_id=((my + d) % N_DEV,),
                device_id_type=pl.DeviceIdType.MESH,
            )

        acc = jnp.zeros((8, n), jnp.float32)
        for cp, off, rows in copies:
            cp.wait()

            def step(i, a, off=off):
                r = pl.multiple_of(off + i * 32, 32)
                blk = xbuf[pl.ds(r, 32), :]
                return a + (
                    (blk[0:8] + blk[8:16]) + (blk[16:24] + blk[24:32])
                )

            acc = lax.fori_loop(0, rows // 32, step, acc)

        comm[my] = jnp.sum(acc, axis=0, keepdims=True)

        pl.semaphore_wait(barrier, N_DEV - 1)
        rdmas = []
        for d in range(1, N_DEV):
            rdma = pltpu.make_async_remote_copy(
                src_ref=comm.at[my],
                dst_ref=comm.at[my],
                send_sem=send_sems.at[d - 1],
                recv_sem=recv_sems.at[d - 1],
                device_id=((my + d) % N_DEV,),
                device_id_type=pl.DeviceIdType.MESH,
            )
            rdma.start()
            rdmas.append(rdma)
        for rdma in rdmas:
            rdma.wait_recv()
        total = (comm[0] + comm[1]) + (comm[2] + comm[3])
        out_ref[...] = total * inv_total
        for rdma in rdmas:
            rdma.wait_send()

    return pl.pallas_call(
        kernel_body,
        out_shape=jax.ShapeDtypeStruct((1, n), jnp.float32),
        in_specs=[pl.BlockSpec(memory_space=pl.ANY)],
        out_specs=pl.BlockSpec(memory_space=pltpu.VMEM),
        scratch_shapes=[
            pltpu.VMEM((m_per, n), jnp.float32),
            pltpu.VMEM((N_DEV, 1, n), jnp.float32),
            pltpu.SemaphoreType.DMA((len(CHUNKS),)),
            pltpu.SemaphoreType.DMA((N_DEV - 1,)),
            pltpu.SemaphoreType.DMA((N_DEV - 1,)),
        ],
        compiler_params=pltpu.CompilerParams(collective_id=0),
    )(x)
```

```python
import jax
import jax.numpy as jnp
from jax import lax
from jax.experimental import pallas as pl
from jax.experimental.pallas import tpu as pltpu

N_DEV = 4
FULL_CHUNKS = (1024, 448)
TAIL_A = (192, 128, 64)
TAIL_B = (320, 64)
W_B = 128
K_RAW = 96
RAW_AFTER_A = 1


def _tree_sum(parts):
    while len(parts) > 1:
        nxt = [parts[i] + parts[i + 1] for i in range(0, len(parts) - 1, 2)]
        if len(parts) % 2:
            nxt.append(parts[-1])
        parts = nxt
    return parts[0]


def _accum(ref, off, rows, acc, unroll):
    u = min(unroll, rows)
    while rows % u:
        u -= 8

    def add_block(start, a):
        blk = ref[pl.ds(start, u), :]
        return a + _tree_sum([blk[8 * g : 8 * g + 8] for g in range(u // 8)])

    if rows == u:
        return add_block(off, acc)
    return lax.fori_loop(
        0,
        rows // u,
        lambda i, a: add_block(pl.multiple_of(off + i * u, 8), a),
        acc,
    )


def _compiler_params():
    try:
        return pltpu.CompilerParams(collective_id=0, disable_semaphore_checks=True)
    except TypeError:
        return pltpu.CompilerParams(collective_id=0)


def pallas_dist_mean_ax0_shard0_i_m2048_n1024_kernel(
x: jax.Array,
):
    m_per, n = x.shape
    n_full = sum(FULL_CHUNKS)
    n_tail = sum(TAIL_A)
    n_local = n_full + n_tail
    assert n_tail == sum(TAIL_B)
    assert n_local + 2 * K_RAW == m_per
    w_a = n - W_B
    inv_total = 1.0 / float(m_per * N_DEV)
    n_copies = len(FULL_CHUNKS) + len(TAIL_A) + len(TAIL_B)
    mesh_id = pl.DeviceIdType.MESH

    def kernel_body(
        x_hbm,
        out_ref,
        buf_full,
        buf_a,
        buf_b,
        buf_raw,
        comm_a,
        comm_b,
        copy_sems,
        send_sems,
        recv_sems,
        raw_send_sems,
        raw_recv_sems,
        ready_sem,
    ):
        n_started = [0]

        def start_copy(src, dst):
            cp = pltpu.make_async_copy(src, dst, copy_sems.at[n_started[0]])
            n_started[0] += 1
            cp.start()
            return cp

        full, part_a, part_b = [], [], []
        off = 0
        for rows in FULL_CHUNKS:
            cp = start_copy(
                x_hbm.at[pl.ds(off, rows)], buf_full.at[pl.ds(off, rows)]
            )
            full.append((cp, off, rows))
            off += rows
        off = 0
        for rows in TAIL_A:
            cp = start_copy(
                x_hbm.at[pl.ds(n_full + off, rows), pl.ds(0, w_a)],
                buf_a.at[pl.ds(off, rows)],
            )
            part_a.append((cp, off, rows))
            off += rows
        off = 0
        for rows in TAIL_B:
            cp = start_copy(
                x_hbm.at[pl.ds(n_full + off, rows), pl.ds(w_a, W_B)],
                buf_b.at[pl.ds(off, rows)],
            )
            part_b.append((cp, off, rows))
            off += rows

        my = lax.axis_index("i")
        right = (my + 1) % N_DEV
        diag = (my + 2) % N_DEV
        left = (my + 3) % N_DEV
        peer = {1: right, 2: diag, 3: left}

        barrier = pltpu.get_barrier_semaphore()
        for nbr in (right, left):
            pl.semaphore_signal(
                barrier, inc=1, device_id=(nbr,), device_id_type=mesh_id
            )
        pl.semaphore_wait(barrier, 2)
        pl.semaphore_signal(
            ready_sem, inc=1, device_id=(left,), device_id_type=mesh_id
        )

        raw = []
        for j, nbr in enumerate((right, left)):
            rc = pltpu.make_async_remote_copy(
                src_ref=x_hbm.at[pl.ds(n_local + j * K_RAW, K_RAW)],
                dst_ref=buf_raw.at[pl.ds(j * K_RAW, K_RAW)],
                send_sem=raw_send_sems.at[j],
                recv_sem=raw_recv_sems.at[j],
                device_id=(nbr,),
                device_id_type=mesh_id,
            )
            rc.start()
            raw.append(rc)

        acc = jnp.zeros((8, n), jnp.float32)
        for cp, off, rows in full:
            cp.wait()
            acc = _accum(buf_full, off, rows, acc, 32)
        acc_a = acc[:, :w_a]
        acc_b = acc[:, w_a:]

        pl.semaphore_wait(ready_sem, 1)

        def send_partial(comm, base):
            rdmas = {}
            for d in (2, 1, 3):
                rdma = pltpu.make_async_remote_copy(
                    src_ref=comm.at[my],
                    dst_ref=comm.at[my],
                    send_sem=send_sems.at[base + d - 1],
                    recv_sem=recv_sems.at[base + d - 1],
                    device_id=(peer[d],),
                    device_id_type=mesh_id,
                )
                rdma.start()
                rdmas[d] = rdma
            return rdmas

        for i, (cp, off, rows) in enumerate(part_a):
            cp.wait()
            acc_a = _accum(buf_a, off, rows, acc_a, 32)
            if i == RAW_AFTER_A:
                for rc in raw:
                    rc.wait_recv()
                acc_r = _accum(
                    buf_raw, 0, 2 * K_RAW, jnp.zeros((8, n), jnp.float32), 32
                )
                acc_a = acc_a + acc_r[:, :w_a]
                acc_b = acc_b + acc_r[:, w_a:]
        comm_a[my] = jnp.sum(acc_a, axis=0, keepdims=True)
        rd_a = send_partial(comm_a, 0)

        for cp, off, rows in part_b:
            cp.wait()
            acc_b = _accum(buf_b, off, rows, acc_b, 512)
        comm_b[my] = jnp.sum(acc_b, axis=0, keepdims=True)
        rd_b = send_partial(comm_b, N_DEV - 1)

        for rc in raw:
            rc.wait_send()
        for rd in (rd_a, rd_b):
            for d in (1, 3, 2):
                rd[d].wait_send()

        for d in (1, 3, 2):
            rd_a[d].wait_recv()
        out_ref[:, pl.ds(0, w_a)] = (
            (comm_a[0] + comm_a[1]) + (comm_a[2] + comm_a[3])
        ) * inv_total
        for d in (1, 3, 2):
            rd_b[d].wait_recv()
        out_ref[:, pl.ds(w_a, W_B)] = (
            (comm_b[0] + comm_b[1]) + (comm_b[2] + comm_b[3])
        ) * inv_total

    return pl.pallas_call(
        kernel_body,
        out_shape=jax.ShapeDtypeStruct((1, n), jnp.float32),
        in_specs=[pl.BlockSpec(memory_space=pl.ANY)],
        out_specs=pl.BlockSpec(memory_space=pltpu.VMEM),
        scratch_shapes=[
            pltpu.VMEM((n_full, n), jnp.float32),
            pltpu.VMEM((n_tail, w_a), jnp.float32),
            pltpu.VMEM((n_tail, W_B), jnp.float32),
            pltpu.VMEM((2 * K_RAW, n), jnp.float32),
            pltpu.VMEM((N_DEV, 1, w_a), jnp.float32),
            pltpu.VMEM((N_DEV, 1, W_B), jnp.float32),
            pltpu.SemaphoreType.DMA((n_copies,)),
            pltpu.SemaphoreType.DMA((2 * (N_DEV - 1),)),
            pltpu.SemaphoreType.DMA((2 * (N_DEV - 1),)),
            pltpu.SemaphoreType.DMA((2,)),
            pltpu.SemaphoreType.DMA((2,)),
            pltpu.SemaphoreType.REGULAR,
        ],
        compiler_params=_compiler_params(),
    )(x)
```

```python
import jax
import jax.numpy as jnp
from jax import lax
from jax.experimental import pallas as pl
from jax.experimental.pallas import tpu as pltpu

N_DEV = 4
FULL_CHUNKS = (1024, 448)
TAIL_A = (192, 128, 64)
TAIL_B = (320, 64)
W_B = 128
K_RAW = 96
RAW_AFTER_A = 1


def _tree_sum(parts):
    while len(parts) > 1:
        nxt = [parts[i] + parts[i + 1] for i in range(0, len(parts) - 1, 2)]
        if len(parts) % 2:
            nxt.append(parts[-1])
        parts = nxt
    return parts[0]


def _accum(ref, off, rows, acc, unroll):
    u = min(unroll, rows)
    while rows % u:
        u -= 8

    def add_block(start, a):
        blk = ref[pl.ds(start, u), :]
        return a + _tree_sum([blk[8 * g : 8 * g + 8] for g in range(u // 8)])

    if rows == u:
        return add_block(off, acc)
    return lax.fori_loop(
        0,
        rows // u,
        lambda i, a: add_block(pl.multiple_of(off + i * u, 8), a),
        acc,
    )


def _compiler_params():
    try:
        return pltpu.CompilerParams(collective_id=0, disable_semaphore_checks=True)
    except TypeError:
        return pltpu.CompilerParams(collective_id=0)


def pallas_dist_mean_ax0_shard0_i_m2048_n1024_kernel(
x: jax.Array,
):
    m_per, n = x.shape
    n_full = sum(FULL_CHUNKS)
    n_tail = sum(TAIL_A)
    n_local = n_full + n_tail
    assert n_tail == sum(TAIL_B)
    assert n_local + 2 * K_RAW == m_per
    w_a = n - W_B
    inv_total = 1.0 / float(m_per * N_DEV)
    n_copies = len(FULL_CHUNKS) + len(TAIL_A) + len(TAIL_B)
    mesh_id = pl.DeviceIdType.MESH

    def kernel_body(
        x_hbm,
        out_ref,
        buf_full,
        buf_a,
        buf_b,
        buf_raw,
        comm_a,
        comm_b,
        copy_sems,
        send_sems,
        recv_sems,
        raw_send_sems,
        raw_recv_sems,
        ready_sem,
    ):
        n_started = [0]

        def start_copy(src, dst):
            cp = pltpu.make_async_copy(src, dst, copy_sems.at[n_started[0]])
            n_started[0] += 1
            cp.start()
            return cp

        full, part_a, part_b = [], [], []
        off = 0
        for c, rows in enumerate(FULL_CHUNKS):
            cp = start_copy(
                x_hbm.at[pl.ds(off, rows)], buf_full.at[pl.ds(off, rows)]
            )
            full.append((cp, off, rows))
            off += rows
            if c == 0:
                my = lax.axis_index("i")
                right = (my + 1) & (N_DEV - 1)
                diag = (my + 2) & (N_DEV - 1)
                left = (my + 3) & (N_DEV - 1)
                barrier = pltpu.get_barrier_semaphore()
                for nbr in (right, left):
                    pl.semaphore_signal(
                        barrier, inc=1, device_id=(nbr,), device_id_type=mesh_id
                    )
        peer = {1: right, 2: diag, 3: left}
        off = 0
        for rows in TAIL_A:
            cp = start_copy(
                x_hbm.at[pl.ds(n_full + off, rows), pl.ds(0, w_a)],
                buf_a.at[pl.ds(off, rows)],
            )
            part_a.append((cp, off, rows))
            off += rows
        off = 0
        for rows in TAIL_B:
            cp = start_copy(
                x_hbm.at[pl.ds(n_full + off, rows), pl.ds(w_a, W_B)],
                buf_b.at[pl.ds(off, rows)],
            )
            part_b.append((cp, off, rows))
            off += rows

        pl.semaphore_wait(barrier, 2)
        pl.semaphore_signal(
            ready_sem, inc=1, device_id=(left,), device_id_type=mesh_id
        )

        raw = []
        for j, nbr in enumerate((right, left)):
            rc = pltpu.make_async_remote_copy(
                src_ref=x_hbm.at[pl.ds(n_local + j * K_RAW, K_RAW)],
                dst_ref=buf_raw.at[pl.ds(j * K_RAW, K_RAW)],
                send_sem=raw_send_sems.at[j],
                recv_sem=raw_recv_sems.at[j],
                device_id=(nbr,),
                device_id_type=mesh_id,
            )
            rc.start()
            raw.append(rc)

        acc = jnp.zeros((8, n), jnp.float32)
        for cp, off, rows in full:
            cp.wait()
            acc = _accum(buf_full, off, rows, acc, 32)
        acc_a = acc[:, :w_a]
        acc_b = acc[:, w_a:]

        pl.semaphore_wait(ready_sem, 1)

        def send_partial(comm, base):
            rdmas = {}
            for d in (2, 1, 3):
                rdma = pltpu.make_async_remote_copy(
                    src_ref=comm.at[my],
                    dst_ref=comm.at[my],
                    send_sem=send_sems.at[base + d - 1],
                    recv_sem=recv_sems.at[base + d - 1],
                    device_id=(peer[d],),
                    device_id_type=mesh_id,
                )
                rdma.start()
                rdmas[d] = rdma
            return rdmas

        for i, (cp, off, rows) in enumerate(part_a):
            cp.wait()
            acc_a = _accum(buf_a, off, rows, acc_a, 32)
            if i == RAW_AFTER_A:
                for rc in raw:
                    rc.wait_recv()
                acc_r = _accum(
                    buf_raw, 0, 2 * K_RAW, jnp.zeros((8, n), jnp.float32), 32
                )
                acc_a = acc_a + acc_r[:, :w_a]
                acc_b = acc_b + acc_r[:, w_a:]
        comm_a[my] = jnp.sum(acc_a, axis=0, keepdims=True)
        rd_a = send_partial(comm_a, 0)

        for cp, off, rows in part_b:
            cp.wait()
            acc_b = _accum(buf_b, off, rows, acc_b, 512)
        comm_b[my] = jnp.sum(acc_b, axis=0, keepdims=True)
        rd_b = send_partial(comm_b, N_DEV - 1)

        for rc in raw:
            rc.wait_send()
        for rd in (rd_a, rd_b):
            for d in (1, 3, 2):
                rd[d].wait_send()

        for d in (1, 3, 2):
            rd_a[d].wait_recv()
        out_ref[:, pl.ds(0, w_a)] = (
            (comm_a[0] + comm_a[1]) + (comm_a[2] + comm_a[3])
        ) * inv_total
        for d in (1, 3, 2):
            rd_b[d].wait_recv()
        out_ref[:, pl.ds(w_a, W_B)] = (
            (comm_b[0] + comm_b[1]) + (comm_b[2] + comm_b[3])
        ) * inv_total

    return pl.pallas_call(
        kernel_body,
        out_shape=jax.ShapeDtypeStruct((1, n), jnp.float32),
        in_specs=[pl.BlockSpec(memory_space=pl.ANY)],
        out_specs=pl.BlockSpec(memory_space=pltpu.VMEM),
        scratch_shapes=[
            pltpu.VMEM((n_full, n), jnp.float32),
            pltpu.VMEM((n_tail, w_a), jnp.float32),
            pltpu.VMEM((n_tail, W_B), jnp.float32),
            pltpu.VMEM((2 * K_RAW, n), jnp.float32),
            pltpu.VMEM((N_DEV, 1, w_a), jnp.float32),
            pltpu.VMEM((N_DEV, 1, W_B), jnp.float32),
            pltpu.SemaphoreType.DMA((n_copies,)),
            pltpu.SemaphoreType.DMA((2 * (N_DEV - 1),)),
            pltpu.SemaphoreType.DMA((2 * (N_DEV - 1),)),
            pltpu.SemaphoreType.DMA((2,)),
            pltpu.SemaphoreType.DMA((2,)),
            pltpu.SemaphoreType.REGULAR,
        ],
        compiler_params=_compiler_params(),
    )(x)
```
